```python
import numpy as np

kernel_name = "dist_argmax_global_i_m4096_n1024"

def setup_inputs():
    return {"x": np.random.randn(16384, 1024).astype(np.float32)}

def reference(x: np.ndarray) -> np.ndarray:
    idx = np.argmax(x, axis=0).astype(np.float32)
    val = np.max(x, axis=0)
    return np.stack([val, idx], axis=0)
```

```python
import jax
import jax.numpy as jnp
from jax import lax
from jax.experimental import pallas as pl
from jax.experimental.pallas import tpu as pltpu

N_DEV = 4
BM = 512
SUB = 8
UNROLL = 8


def _better(x, m):
    return jnp.logical_and(jnp.logical_not(x <= m), m == m)


def pallas_dist_argmax_global_i_m4096_n1024_kernel(
x: jax.Array,
):
    m_per, n = x.shape
    nsteps = m_per // BM
    groups = BM // SUB

    def body(x_ref, out_ref, accv_ref, acci_ref, comm_ref, send_sems, recv_sems):
        step = pl.program_id(0)
        my = lax.axis_index("i")

        @pl.when(step == 0)
        def _():
            barrier = pltpu.get_barrier_semaphore()
            for k in range(1, N_DEV):
                pl.semaphore_signal(
                    barrier, inc=1,
                    device_id=((my + k) % N_DEV,),
                    device_id_type=pl.DeviceIdType.MESH,
                )
            accv_ref[...] = jnp.full((SUB, n), -jnp.inf, jnp.float32)
            acci_ref[...] = jnp.zeros((SUB, n), jnp.float32)

        g0 = step * groups

        def inner(g, carry):
            mv, mi = carry
            xt = x_ref[pl.ds(pl.multiple_of(g * SUB, SUB), SUB), :]
            upd = _better(xt, mv)
            mv = jnp.where(upd, xt, mv)
            mi = jnp.where(upd, (g0 + g).astype(jnp.float32), mi)
            return mv, mi

        mv, mi = lax.fori_loop(
            0, groups, inner, (accv_ref[...], acci_ref[...]), unroll=UNROLL
        )
        accv_ref[...] = mv
        acci_ref[...] = mi

        @pl.when(step == nsteps - 1)
        def _():
            sub_iota = lax.broadcasted_iota(jnp.int32, (SUB, n), 0)
            rows = mi * float(SUB) + (sub_iota + my * m_per).astype(jnp.float32)
            isn = mv != mv
            any_nan = jnp.max(jnp.where(isn, 1.0, 0.0), axis=0, keepdims=True) > 0.0
            mx = jnp.max(jnp.where(isn, -jnp.inf, mv), axis=0, keepdims=True)
            hit = jnp.logical_or(
                isn, jnp.logical_and(jnp.logical_not(any_nan), mv == mx))
            idx = jnp.min(jnp.where(hit, rows, jnp.float32(3.0e38)),
                          axis=0, keepdims=True)
            val = jnp.where(any_nan, jnp.float32(jnp.nan), mx)
            comm_ref[my, 0:1, :] = val
            comm_ref[my, 1:2, :] = idx

            barrier = pltpu.get_barrier_semaphore()
            pl.semaphore_wait(barrier, N_DEV - 1)
            copies = []
            for k in range(1, N_DEV):
                c = pltpu.make_async_remote_copy(
                    src_ref=comm_ref.at[my],
                    dst_ref=comm_ref.at[my],
                    send_sem=send_sems.at[k - 1],
                    recv_sem=recv_sems.at[k - 1],
                    device_id=((my + k) % N_DEV,),
                    device_id_type=pl.DeviceIdType.MESH,
                )
                c.start()
                copies.append(c)
            for c in copies:
                c.wait_send()
            for k in range(1, N_DEV):
                src = (my - k) % N_DEV
                pltpu.make_async_remote_copy(
                    src_ref=comm_ref.at[src],
                    dst_ref=comm_ref.at[src],
                    send_sem=send_sems.at[k - 1],
                    recv_sem=recv_sems.at[k - 1],
                    device_id=(src,),
                    device_id_type=pl.DeviceIdType.MESH,
                ).wait_recv()

            bv = comm_ref[0, 0:1, :]
            bi = comm_ref[0, 1:2, :]
            for d in range(1, N_DEV):
                v = comm_ref[d, 0:1, :]
                i = comm_ref[d, 1:2, :]
                upd = _better(v, bv)
                bv = jnp.where(upd, v, bv)
                bi = jnp.where(upd, i, bi)
            out_ref[0:1, :] = bv
            out_ref[1:2, :] = bi

    return pl.pallas_call(
        body,
        grid=(nsteps,),
        in_specs=[pl.BlockSpec((BM, n), lambda i: (i, 0))],
        out_specs=pl.BlockSpec((2, n), lambda i: (0, 0)),
        out_shape=jax.ShapeDtypeStruct((2, n), jnp.float32),
        scratch_shapes=[
            pltpu.VMEM((SUB, n), jnp.float32),
            pltpu.VMEM((SUB, n), jnp.float32),
            pltpu.VMEM((N_DEV, 2, n), jnp.float32),
            pltpu.SemaphoreType.DMA((N_DEV - 1,)),
            pltpu.SemaphoreType.DMA((N_DEV - 1,)),
        ],
        compiler_params=pltpu.CompilerParams(
            collective_id=0,
            dimension_semantics=("arbitrary",),
        ),
    )(x)
```

```python
import jax
import jax.numpy as jnp
from jax import lax
from jax.experimental import pallas as pl
from jax.experimental.pallas import tpu as pltpu

N_DEV = 4
CH = 128
NBUF = 8
SUB = 8


def _better(x, m):
    return jnp.logical_and(jnp.logical_not(x <= m), m == m)


def pallas_dist_argmax_global_i_m4096_n1024_kernel(
x: jax.Array,
):
    m_per, n = x.shape
    nch = m_per // CH
    groups = CH // SUB

    def body(x_hbm, out_ref, buf, comm_ref, ld_sems, send_sems, recv_sems):
        my = lax.axis_index("i")

        def load(c, slot):
            return pltpu.make_async_copy(
                x_hbm.at[pl.ds(pl.multiple_of(c * CH, CH), CH), :],
                buf.at[slot], ld_sems.at[slot])

        for s in range(NBUF):
            load(s, s).start()

        barrier = pltpu.get_barrier_semaphore()
        for k in range(1, N_DEV):
            pl.semaphore_signal(
                barrier, inc=1,
                device_id=((my + k) % N_DEV,),
                device_id_type=pl.DeviceIdType.MESH,
            )

        def chunk(c, carry):
            mv, mi = carry
            slot = c % NBUF
            load(c, slot).wait()
            for g in range(groups):
                xt = buf[slot, g * SUB:(g + 1) * SUB, :]
                upd = _better(xt, mv)
                mv = jnp.where(upd, xt, mv)
                mi = jnp.where(upd, (c * groups + g).astype(jnp.float32), mi)

            @pl.when(c + NBUF < nch)
            def _():
                load(c + NBUF, slot).start()

            return mv, mi

        mv, mi = lax.fori_loop(
            0, nch, chunk,
            (jnp.full((SUB, n), -jnp.inf, jnp.float32),
             jnp.zeros((SUB, n), jnp.float32)),
        )

        sub_iota = lax.broadcasted_iota(jnp.int32, (SUB, n), 0)
        rows = mi * float(SUB) + (sub_iota + my * m_per).astype(jnp.float32)
        isn = mv != mv
        any_nan = jnp.max(jnp.where(isn, 1.0, 0.0), axis=0, keepdims=True) > 0.0
        mx = jnp.max(jnp.where(isn, -jnp.inf, mv), axis=0, keepdims=True)
        hit = jnp.logical_or(
            isn, jnp.logical_and(jnp.logical_not(any_nan), mv == mx))
        idx = jnp.min(jnp.where(hit, rows, jnp.float32(3.0e38)),
                      axis=0, keepdims=True)
        val = jnp.where(any_nan, jnp.float32(jnp.nan), mx)
        comm_ref[my, 0:1, :] = val
        comm_ref[my, 1:2, :] = idx

        pl.semaphore_wait(barrier, N_DEV - 1)
        copies = []
        for k in range(1, N_DEV):
            cp = pltpu.make_async_remote_copy(
                src_ref=comm_ref.at[my],
                dst_ref=comm_ref.at[my],
                send_sem=send_sems.at[k - 1],
                recv_sem=recv_sems.at[k - 1],
                device_id=((my + k) % N_DEV,),
                device_id_type=pl.DeviceIdType.MESH,
            )
            cp.start()
            copies.append(cp)
        for k in range(1, N_DEV):
            src = (my - k) % N_DEV
            pltpu.make_async_remote_copy(
                src_ref=comm_ref.at[src],
                dst_ref=comm_ref.at[src],
                send_sem=send_sems.at[k - 1],
                recv_sem=recv_sems.at[k - 1],
                device_id=(src,),
                device_id_type=pl.DeviceIdType.MESH,
            ).wait_recv()

        bv = comm_ref[0, 0:1, :]
        bi = comm_ref[0, 1:2, :]
        for d in range(1, N_DEV):
            v = comm_ref[d, 0:1, :]
            i = comm_ref[d, 1:2, :]
            upd = _better(v, bv)
            bv = jnp.where(upd, v, bv)
            bi = jnp.where(upd, i, bi)
        out_ref[0:1, :] = bv
        out_ref[1:2, :] = bi

        for cp in copies:
            cp.wait_send()

    return pl.pallas_call(
        body,
        in_specs=[pl.BlockSpec(memory_space=pl.ANY)],
        out_specs=pl.BlockSpec(memory_space=pltpu.VMEM),
        out_shape=jax.ShapeDtypeStruct((2, n), jnp.float32),
        scratch_shapes=[
            pltpu.VMEM((NBUF, CH, n), jnp.float32),
            pltpu.VMEM((N_DEV, 2, n), jnp.float32),
            pltpu.SemaphoreType.DMA((NBUF,)),
            pltpu.SemaphoreType.DMA((N_DEV - 1,)),
            pltpu.SemaphoreType.DMA((N_DEV - 1,)),
        ],
        compiler_params=pltpu.CompilerParams(collective_id=0),
    )(x)
```
